```python
import numpy as np

kernel_name = "dist_moe_cap_ep_outshard_n2048_d512_e8_h1024"

def setup_inputs():
    x = np.random.randn(2048, 512).astype(np.float32)
    router_W = np.random.randn(512, 32).astype(np.float32) * 0.1
    scores64 = x.astype(np.float64) @ router_W.astype(np.float64)
    route_idx = np.argsort(-scores64, axis=-1)[:, :1].astype(np.int32)
    expert_W = np.random.randn(32, 512, 1024).astype(np.float32) * 0.02
    return {"x": x, "router_W": router_W, "route_idx": route_idx, "expert_W": expert_W}

def reference(x, router_W, route_idx, expert_W):
    counts = np.zeros(32, dtype=np.int64)
    out = np.zeros((2048, 1024), dtype=np.float32)
    for i in range(2048):
        e = int(route_idx[i, 0])
        if counts[e] < 51:
            out[i] = x[i] @ expert_W[e]
            counts[e] += 1
    return out
```

```python
import jax
import jax.numpy as jnp
from jax import lax
from jax.experimental import pallas as pl
from jax.experimental.pallas import tpu as pltpu

N, D, H = 2048, 512, 1024
NE, EL, NDEV = 32, 8, 4
CAP, SL = 51, 64
TOK = N // NDEV
NB = N // 128
HW = H // 2
OC = 64


def _dyn_wait(buf, sem, n, hi_bit):
    bit = hi_bit
    while bit >= 8:
        @pl.when((n & bit) != 0)
        def _(bit=bit):
            pltpu.make_async_copy(buf.at[pl.ds(0, bit)], buf.at[pl.ds(0, bit)], sem).wait()
        bit //= 2

    @pl.loop(0, n & 7)
    def _(i):
        pltpu.make_async_copy(buf.at[pl.ds(0, 1)], buf.at[pl.ds(0, 1)], sem).wait()


def _dyn_pad(src, trash, sem, n):
    bit = TOK
    while bit >= 8:
        @pl.when((n & bit) != 0)
        def _(bit=bit):
            pltpu.make_async_copy(src.at[pl.ds(0, bit)], trash.at[pl.ds(bit, bit)], sem).start()
        bit //= 2

    @pl.loop(0, n & 7)
    def _(i):
        pltpu.make_async_copy(src.at[pl.ds(0, 1)], trash.at[pl.ds(i, 1)], sem).start()


def body(x_hbm, r_hbm, w_hbm, o_hbm,
         wbuf, xbuf, ybuf, stage, obuf, zbuf, trash, rbuf, tab_v, tab_s,
         wsem, xsem, ssem, rsem, osem, msem):
    me = lax.axis_index("i")
    rcp = pltpu.make_async_copy(r_hbm, rbuf, msem.at[0])
    rcp.start()
    wcp = [pltpu.make_async_copy(w_hbm.at[j], wbuf.at[j], wsem.at[j]) for j in range(EL)]
    for c in wcp[:2]:
        c.start(priority=1)

    stage[...] = jnp.zeros(stage.shape, jnp.uint32)
    zbuf[...] = jnp.zeros(zbuf.shape, jnp.uint32)
    bar = pltpu.get_barrier_semaphore()
    for k in range(1, NDEV):
        pl.semaphore_signal(bar, 1, device_id=(me + k) % NDEV,
                            device_id_type=pl.DeviceIdType.LOGICAL)

    ri = lax.broadcasted_iota(jnp.int32, (128, 256), 0)
    ci = lax.broadcasted_iota(jnp.int32, (128, 256), 1)
    u1 = jnp.where((ri <= ci), 1.0, 0.0).astype(jnp.bfloat16)
    rcp.wait()
    r = rbuf[...]
    eid = lax.broadcasted_iota(jnp.int32, (NE, 128), 0)
    lane = lax.broadcasted_iota(jnp.int32, (NE, 128), 1)
    oh = [r[b:b + 1, :] == eid for b in range(NB)]
    es = jnp.concatenate([jnp.where(m, 1.0, 0.0) for m in oh], axis=0).astype(jnp.bfloat16)
    cs = jnp.dot(es, u1, preferred_element_type=jnp.float32)
    sid = lax.broadcasted_iota(jnp.int32, (SL, 128), 0).astype(jnp.float32)
    lanef = lane.astype(jnp.float32)
    pre = jnp.zeros((NE, 128), jnp.float32)
    kept = jnp.zeros((1, 128), jnp.float32)
    lhs, rhs = [], []
    for b in range(NB):
        blk = cs[b * NE:(b + 1) * NE]
        pos = jnp.sum(jnp.where(oh[b], blk[:, :128] + pre, 0.0), axis=0, keepdims=True) - 1.0
        pre = pre + blk[:, 128:]
        rhs.append(jnp.where(pos == sid, 1.0, 0.0).astype(jnp.bfloat16))
        lhs.append(jnp.concatenate(
            [jnp.where(oh[b], lanef, 0.0), jnp.where(oh[b], float(b), 0.0)],
            axis=0).astype(jnp.bfloat16))
        ok = (pos >= 0.0) & (pos < float(CAP)) & (me == b // 4)
        kept = kept + jnp.where(ok, 1.0, 0.0)
    tk = lax.dot_general(jnp.concatenate(lhs, axis=1), jnp.concatenate(rhs, axis=1),
                         (((1,), (1,)), ((), ())), preferred_element_type=jnp.float32)
    tok = tk[:NE] + 128.0 * tk[NE:]
    tok = jnp.concatenate([tok, jnp.zeros((NE, 128 - SL), jnp.float32)], axis=1)
    nkept = jnp.sum(kept, axis=1, keepdims=True)
    tab = jnp.where(lane == 126, jnp.minimum(pre, float(CAP)), tok)
    tab = jnp.where(lane == 127, nkept, tab)
    tab_v[...] = tab.astype(jnp.int32)
    tcp = pltpu.make_async_copy(tab_v.at[pl.ds(pl.multiple_of(me * EL, EL), EL)], tab_s, msem.at[1])
    tcp.start()
    tcp.wait()

    def gather(j):
        @pl.loop(0, CAP)
        def _(s):
            pltpu.make_async_copy(x_hbm.at[pl.ds(tab_s[j, s], 1)],
                                  xbuf.at[pl.ds(j * SL + s, 1)], xsem.at[j]).start()

    gather(0)
    gather(1)
    _dyn_pad(zbuf, trash, rsem, TOK - tab_s[0, 127])

    nsent = 0
    for j in range(EL):
        pltpu.make_async_copy(xbuf.at[pl.ds(0, 48)], xbuf.at[pl.ds(0, 48)], xsem.at[j]).wait()
        for _ in range(CAP - 48):
            pltpu.make_async_copy(xbuf.at[pl.ds(0, 1)], xbuf.at[pl.ds(0, 1)], xsem.at[j]).wait()
        wcp[j].wait()
        if j + 2 < EL:
            wcp[j + 2].start(priority=1)
        xv = xbuf[j * SL:(j + 1) * SL, :].astype(jnp.bfloat16)
        y = jnp.dot(xv, wbuf[j].astype(jnp.bfloat16), preferred_element_type=jnp.float32)
        yb = pltpu.bitcast(y.astype(jnp.bfloat16).astype(jnp.float32), jnp.uint32)
        ybuf[j * SL:(j + 1) * SL, :] = yb[:, :HW] | (yb[:, HW:] >> 16)
        if j == 0:
            pl.semaphore_wait(bar, NDEV - 1)
        n = tab_s[j, 126]
        nsent = nsent + n

        @pl.loop(0, n)
        def _(s):
            t = tab_s[j, s]
            pltpu.make_async_remote_copy(
                ybuf.at[pl.ds(j * SL + s, 1)], stage.at[pl.ds(t & (TOK - 1), 1)],
                ssem, rsem, device_id=t >> 9,
                device_id_type=pl.DeviceIdType.LOGICAL).start()

        if j + 2 < EL:
            gather(j + 2)

    pltpu.make_async_copy(stage, stage, rsem).wait()
    for c in range(TOK // OC):
        rows = pl.ds(c * OC, OC)
        v = stage[rows, :]
        obuf[rows, :HW] = pltpu.bitcast(v & jnp.uint32(0xFFFF0000), jnp.float32)
        obuf[rows, HW:] = pltpu.bitcast(v << 16, jnp.float32)
        pltpu.make_async_copy(obuf.at[rows], o_hbm.at[rows], osem).start()
    _dyn_wait(ybuf, ssem, nsent, 256)
    pltpu.make_async_copy(obuf, o_hbm, osem).wait()


def pallas_dist_moe_cap_ep_outshard_n2048_d512_e8_h1024_kernel(x, router_W, route_idx, expert_W):
    del router_W
    r = route_idx.astype(jnp.int32).reshape(NB, 128)
    any_spec = pl.BlockSpec(memory_space=pltpu.HBM)
    dma = pltpu.SemaphoreType.DMA
    return pl.pallas_call(
        body,
        out_shape=jax.ShapeDtypeStruct((TOK, H), jnp.float32),
        in_specs=[any_spec] * 3,
        out_specs=any_spec,
        scratch_shapes=[
            pltpu.VMEM((EL, D, H), jnp.float32),
            pltpu.VMEM((EL * SL, D), jnp.float32),
            pltpu.VMEM((EL * SL, HW), jnp.uint32),
            pltpu.VMEM((TOK, HW), jnp.uint32),
            pltpu.VMEM((TOK, H), jnp.float32),
            pltpu.VMEM((TOK, HW), jnp.uint32),
            pltpu.VMEM((2 * TOK, HW), jnp.uint32),
            pltpu.VMEM((NB, 128), jnp.int32),
            pltpu.VMEM((NE, 128), jnp.int32),
            pltpu.SMEM((EL, 128), jnp.int32),
            dma((EL,)), dma((EL,)), dma, dma, dma, dma((2,)),
        ],
        compiler_params=pltpu.CompilerParams(collective_id=0, vmem_limit_bytes=64 << 20),
    )(x, r, expert_W)
```

```python
import jax
import jax.numpy as jnp
from jax import lax
from jax.experimental import pallas as pl
from jax.experimental.pallas import tpu as pltpu

N, D, H = 2048, 512, 1024
NE, EL, NDEV = 32, 8, 4
CAP, SL = 51, 64
TOK = N // NDEV
NB = N // 128
HW = H // 2


def _dyn_wait(buf, sem, n, hi_bit):
    bit = hi_bit
    while bit >= 8:
        @pl.when((n & bit) != 0)
        def _(bit=bit):
            pltpu.make_async_copy(buf.at[pl.ds(0, bit)], buf.at[pl.ds(0, bit)], sem).wait()
        bit //= 2

    @pl.loop(0, n & 7)
    def _(i):
        pltpu.make_async_copy(buf.at[pl.ds(0, 1)], buf.at[pl.ds(0, 1)], sem).wait()


def _dyn_pad(src, trash, sem, n):
    bit = TOK
    while bit >= 8:
        @pl.when((n & bit) != 0)
        def _(bit=bit):
            pltpu.make_async_copy(src.at[pl.ds(0, bit)], trash.at[pl.ds(bit, bit)], sem).start()
        bit //= 2

    @pl.loop(0, n & 7)
    def _(i):
        pltpu.make_async_copy(src.at[pl.ds(0, 1)], trash.at[pl.ds(i, 1)], sem).start()


def body(x_hbm, r_hbm, w_hbm, o_ref,
         wbuf, xbuf, ybuf, stage, zbuf, trash, rbuf, tab_v, tab_s,
         wsem, xsem, ssem, rsem, msem):
    me = lax.axis_index("i")
    rcp = pltpu.make_async_copy(r_hbm, rbuf, msem.at[0])
    rcp.start()
    wcp = [pltpu.make_async_copy(w_hbm.at[j], wbuf.at[j], wsem.at[j]) for j in range(EL)]
    for c in wcp[:2]:
        c.start(priority=1)

    stage[...] = jnp.zeros(stage.shape, jnp.uint32)
    zbuf[...] = jnp.zeros(zbuf.shape, jnp.uint32)
    bar = pltpu.get_barrier_semaphore()
    for k in range(1, NDEV):
        pl.semaphore_signal(bar, 1, device_id=(me + k) % NDEV,
                            device_id_type=pl.DeviceIdType.LOGICAL)

    ri = lax.broadcasted_iota(jnp.int32, (128, 256), 0)
    ci = lax.broadcasted_iota(jnp.int32, (128, 256), 1)
    u1 = jnp.where((ri <= ci), 1.0, 0.0).astype(jnp.bfloat16)
    rcp.wait()
    r = rbuf[...]
    eid = lax.broadcasted_iota(jnp.int32, (NE, 128), 0)
    lane = lax.broadcasted_iota(jnp.int32, (NE, 128), 1)
    oh = [r[b:b + 1, :] == eid for b in range(NB)]
    es = jnp.concatenate([jnp.where(m, 1.0, 0.0) for m in oh], axis=0).astype(jnp.bfloat16)
    cs = jnp.dot(es, u1, preferred_element_type=jnp.float32)
    sid = lax.broadcasted_iota(jnp.int32, (SL, 128), 0).astype(jnp.float32)
    lanef = lane.astype(jnp.float32)
    pre = jnp.zeros((NE, 128), jnp.float32)
    kept = jnp.zeros((1, 128), jnp.float32)
    lhs, rhs = [], []
    for b in range(NB):
        blk = cs[b * NE:(b + 1) * NE]
        pos = jnp.sum(jnp.where(oh[b], blk[:, :128] + pre, 0.0), axis=0, keepdims=True) - 1.0
        pre = pre + blk[:, 128:]
        rhs.append(jnp.where(pos == sid, 1.0, 0.0).astype(jnp.bfloat16))
        lhs.append(jnp.concatenate(
            [jnp.where(oh[b], lanef, 0.0), jnp.where(oh[b], float(b), 0.0)],
            axis=0).astype(jnp.bfloat16))
        ok = (pos >= 0.0) & (pos < float(CAP)) & (me == b // 4)
        kept = kept + jnp.where(ok, 1.0, 0.0)
    tk = lax.dot_general(jnp.concatenate(lhs, axis=1), jnp.concatenate(rhs, axis=1),
                         (((1,), (1,)), ((), ())), preferred_element_type=jnp.float32)
    tok = tk[:NE] + 128.0 * tk[NE:]
    tok = jnp.concatenate([tok, jnp.zeros((NE, 128 - SL), jnp.float32)], axis=1)
    nkept = jnp.sum(kept, axis=1, keepdims=True)
    tab = jnp.where(lane == 126, jnp.minimum(pre, float(CAP)), tok)
    tab = jnp.where(lane == 127, nkept, tab)
    tab_v[...] = tab.astype(jnp.int32)
    tcp = pltpu.make_async_copy(tab_v.at[pl.ds(pl.multiple_of(me * EL, EL), EL)], tab_s, msem.at[1])
    tcp.start()
    tcp.wait()

    def gather(j):
        @pl.loop(0, CAP)
        def _(s):
            pltpu.make_async_copy(x_hbm.at[pl.ds(tab_s[j, s], 1)],
                                  xbuf.at[pl.ds(j * SL + s, 1)], xsem.at[j]).start()

    gather(0)
    gather(1)
    _dyn_pad(zbuf, trash, rsem, TOK - tab_s[0, 127])

    nsent = 0
    for j in range(EL):
        pltpu.make_async_copy(xbuf.at[pl.ds(0, 48)], xbuf.at[pl.ds(0, 48)], xsem.at[j]).wait()
        for _ in range(CAP - 48):
            pltpu.make_async_copy(xbuf.at[pl.ds(0, 1)], xbuf.at[pl.ds(0, 1)], xsem.at[j]).wait()
        wcp[j].wait()
        if j + 2 < EL:
            wcp[j + 2].start(priority=1)
        xv = xbuf[j * SL:(j + 1) * SL, :].astype(jnp.bfloat16)
        y = jnp.dot(xv, wbuf[j].astype(jnp.bfloat16), preferred_element_type=jnp.float32)
        yb = pltpu.bitcast(y.astype(jnp.bfloat16).astype(jnp.float32), jnp.uint32)
        ybuf[j * SL:(j + 1) * SL, :] = yb[:, :HW] | (yb[:, HW:] >> 16)
        if j == 0:
            pl.semaphore_wait(bar, NDEV - 1)
        n = tab_s[j, 126]
        nsent = nsent + n

        @pl.loop(0, n)
        def _(s):
            t = tab_s[j, s]
            pltpu.make_async_remote_copy(
                ybuf.at[pl.ds(j * SL + s, 1)], stage.at[pl.ds(t & (TOK - 1), 1)],
                ssem, rsem, device_id=t >> 9,
                device_id_type=pl.DeviceIdType.LOGICAL).start()

        if j + 2 < EL:
            gather(j + 2)

    pltpu.make_async_copy(stage, stage, rsem).wait()
    v = stage[...]
    o_ref[:, :HW] = pltpu.bitcast(v & jnp.uint32(0xFFFF0000), jnp.float32)
    o_ref[:, HW:] = pltpu.bitcast(v << 16, jnp.float32)
    _dyn_wait(ybuf, ssem, nsent, 256)


def pallas_dist_moe_cap_ep_outshard_n2048_d512_e8_h1024_kernel(x, router_W, route_idx, expert_W):
    del router_W
    r = route_idx.astype(jnp.int32).reshape(NB, 128)
    any_spec = pl.BlockSpec(memory_space=pltpu.HBM)
    dma = pltpu.SemaphoreType.DMA
    return pl.pallas_call(
        body,
        out_shape=pltpu.VMEM((TOK, H), jnp.float32),
        in_specs=[any_spec] * 3,
        out_specs=pl.BlockSpec(memory_space=pltpu.VMEM),
        scratch_shapes=[
            pltpu.VMEM((EL, D, H), jnp.float32),
            pltpu.VMEM((EL * SL, D), jnp.float32),
            pltpu.VMEM((EL * SL, HW), jnp.uint32),
            pltpu.VMEM((TOK, HW), jnp.uint32),
            pltpu.VMEM((TOK, HW), jnp.uint32),
            pltpu.VMEM((2 * TOK, HW), jnp.uint32),
            pltpu.VMEM((NB, 128), jnp.int32),
            pltpu.VMEM((NE, 128), jnp.int32),
            pltpu.SMEM((EL, 128), jnp.int32),
            dma((EL,)), dma((EL,)), dma, dma, dma((2,)),
        ],
        compiler_params=pltpu.CompilerParams(collective_id=0, vmem_limit_bytes=64 << 20),
    )(x, r, expert_W)
```
